```python
import numpy as np

kernel_name = "dist_mean_ax0_shard0_i_m4096_n1024"

def setup_inputs():
    return {"x": np.random.randn(16384, 1024).astype(np.float32)}

def reference(x: np.ndarray) -> np.ndarray:
    return np.mean(x, axis=0, keepdims=True)
```

```python
import jax
import jax.numpy as jnp
from jax import lax
from jax.experimental import pallas as pl
from jax.experimental.pallas import tpu as pltpu

N_DEV = 4


def pallas_dist_mean_ax0_shard0_i_m4096_n1024_kernel(x: jax.Array):
    m_per, n = x.shape
    chunk = 256
    n_chunks = m_per // chunk
    depth = 4
    inv_total = 1.0 / (m_per * N_DEV)

    def body(x_hbm, out_ref, buf, comm, copy_sems, send_sems, recv_sems):
        my = lax.axis_index("i")

        def copy(c):
            return pltpu.make_async_copy(
                x_hbm.at[pl.ds(c * chunk, chunk), :],
                buf.at[pl.ds(c * chunk, chunk), :],
                copy_sems.at[c],
            )

        for c in range(depth):
            copy(c).start()

        barrier = pltpu.get_barrier_semaphore()
        for d in range(1, N_DEV):
            pl.semaphore_signal(
                barrier, inc=1,
                device_id=((my + d) % N_DEV,),
                device_id_type=pl.DeviceIdType.MESH,
            )

        acc = jnp.zeros((8, n), jnp.float32)
        for c in range(n_chunks):
            copy(c).wait()
            if c + depth < n_chunks:
                copy(c + depth).start()
            blk = buf[pl.ds(c * chunk, chunk), :]
            acc = acc + jnp.sum(blk.reshape(chunk // 8, 8, n), axis=0)
        comm[0] = jnp.sum(acc, axis=0, keepdims=True)

        pl.semaphore_wait(barrier, N_DEV - 1)

        rdmas = []
        for d in range(1, N_DEV):
            rdma = pltpu.make_async_remote_copy(
                src_ref=comm.at[0],
                dst_ref=comm.at[d],
                send_sem=send_sems.at[d - 1],
                recv_sem=recv_sems.at[d - 1],
                device_id=((my + d) % N_DEV,),
                device_id_type=pl.DeviceIdType.MESH,
            )
            rdma.start()
            rdmas.append(rdma)
        for rdma in rdmas:
            rdma.wait_recv()
        total = (comm[0] + comm[1]) + (comm[2] + comm[3])
        out_ref[...] = total * inv_total
        for rdma in rdmas:
            rdma.wait_send()

    return pl.pallas_call(
        body,
        out_shape=jax.ShapeDtypeStruct((1, n), jnp.float32),
        in_specs=[pl.BlockSpec(memory_space=pl.ANY)],
        out_specs=pl.BlockSpec(memory_space=pltpu.VMEM),
        scratch_shapes=[
            pltpu.VMEM((m_per, n), jnp.float32),
            pltpu.VMEM((N_DEV, 1, n), jnp.float32),
            pltpu.SemaphoreType.DMA((n_chunks,)),
            pltpu.SemaphoreType.DMA((N_DEV - 1,)),
            pltpu.SemaphoreType.DMA((N_DEV - 1,)),
        ],
        compiler_params=pltpu.CompilerParams(
            collective_id=0, vmem_limit_bytes=40 * 1024 * 1024
        ),
    )(x)
```

```python
import jax
import jax.numpy as jnp
from jax import lax
from jax.experimental import pallas as pl
from jax.experimental.pallas import tpu as pltpu

N_DEV = 4
MESH = pl.DeviceIdType.MESH

RAW_ROWS = 208
SPLIT_ROWS = 160
LANE = 128
BIG_CHUNK = 512
TAIL_CHUNKS = (256, 128, 64, 32, 16, 16)
RAW_WAIT_BACK = 4


def _pieces(rows_local, n):
    wide_cols = n - LANE
    split0 = rows_local - SPLIT_ROWS
    sizes, rest = [], split0 - sum(TAIL_CHUNKS)
    while rest > 0:
        sizes.append(min(BIG_CHUNK, rest))
        rest -= sizes[-1]
    sizes += list(TAIL_CHUNKS)
    pieces = [(split0, SPLIT_ROWS, 0, wide_cols)]
    row = 0
    for size in sizes:
        pieces.append((row, size, 0, n))
        row += size
    pieces.append((split0, SPLIT_ROWS, wide_cols, LANE))
    return pieces


def _colsum8(v):
    return jnp.sum(v.reshape(v.shape[0] // 8, 8, v.shape[1]), axis=0)


def pallas_dist_mean_ax0_shard0_i_m4096_n1024_kernel(x: jax.Array):
    m_per, n = x.shape
    rows_local = m_per - 2 * RAW_ROWS
    wide_cols = n - LANE
    pieces = _pieces(rows_local, n)
    n_pieces = len(pieces)
    last_wide = n_pieces - 2
    inv_rows = 1.0 / (m_per * N_DEV)

    def body(x_hbm, out_ref, buf, raw_buf, comm,
             copy_sems, raw_send_sems, raw_recv_sems, send_sems, recv_sems):
        my = lax.axis_index("i")

        def peer(d):
            return ((my + d) % N_DEV,)

        def local_copy(p):
            r0, rn, c0, cn = pieces[p]
            return pltpu.make_async_copy(
                x_hbm.at[pl.ds(r0, rn), pl.ds(c0, cn)],
                buf.at[pl.ds(r0, rn), pl.ds(c0, cn)],
                copy_sems.at[p],
            )

        def partial_msg(d, k, c0, cn):
            return pltpu.make_async_remote_copy(
                src_ref=comm.at[0, :, pl.ds(c0, cn)],
                dst_ref=comm.at[d, :, pl.ds(c0, cn)],
                send_sem=send_sems.at[k],
                recv_sem=recv_sems.at[k],
                device_id=peer(d),
                device_id_type=MESH,
            )

        local_copy(0).start()
        barrier = pltpu.get_barrier_semaphore()
        for d in (1, 3, 2):
            pl.semaphore_signal(barrier, inc=1, device_id=peer(d), device_id_type=MESH)
        for p in range(1, n_pieces):
            local_copy(p).start()
        pl.semaphore_wait(barrier, N_DEV - 1)

        raw = []
        for b, d in enumerate((1, 3)):
            rd = pltpu.make_async_remote_copy(
                src_ref=x_hbm.at[pl.ds(rows_local + b * RAW_ROWS, RAW_ROWS), :],
                dst_ref=raw_buf.at[b],
                send_sem=raw_send_sems.at[b],
                recv_sem=raw_recv_sems.at[b],
                device_id=peer(d),
                device_id_type=MESH,
            )
            rd.start()
            raw.append(rd)

        to_next = partial_msg(1, 0, 0, n)
        to_prev = partial_msg(3, 1, 0, n)
        to_diag_wide = partial_msg(2, 2, 0, wide_cols)
        to_diag_last = partial_msg(2, 3, wide_cols, LANE)

        acc_wide = jnp.zeros((8, wide_cols), jnp.float32)
        acc_last = jnp.zeros((8, LANE), jnp.float32)
        for p, (r0, rn, c0, cn) in enumerate(pieces):
            local_copy(p).wait()
            if c0 == 0:
                acc_wide += _colsum8(buf[pl.ds(r0, rn), pl.ds(0, wide_cols)])
            if c0 + cn == n:
                acc_last += _colsum8(buf[pl.ds(r0, rn), pl.ds(wide_cols, LANE)])
            if p == last_wide - RAW_WAIT_BACK:
                for b, rd in enumerate(raw):
                    rd.wait_recv()
                    acc_wide += _colsum8(raw_buf[b, :, pl.ds(0, wide_cols)])
                    acc_last += _colsum8(raw_buf[b, :, pl.ds(wide_cols, LANE)])
                for rd in raw:
                    rd.wait_send()
            if p == last_wide:
                comm[0, :, pl.ds(0, wide_cols)] = jnp.sum(acc_wide, axis=0, keepdims=True)
                to_diag_wide.start()
        comm[0, :, pl.ds(wide_cols, LANE)] = jnp.sum(acc_last, axis=0, keepdims=True)
        to_diag_last.start()
        to_next.start()
        to_prev.start()

        for msg in (to_diag_wide, to_diag_last, to_next, to_prev):
            msg.wait_send()
        to_next.wait_recv()
        to_prev.wait_recv()
        near = (comm[0] + comm[1]) + comm[3]
        to_diag_wide.wait_recv()
        to_diag_last.wait_recv()
        out_ref[...] = (near + comm[2]) * inv_rows

    return pl.pallas_call(
        body,
        out_shape=jax.ShapeDtypeStruct((1, n), jnp.float32),
        in_specs=[pl.BlockSpec(memory_space=pl.ANY)],
        out_specs=pl.BlockSpec(memory_space=pltpu.VMEM),
        scratch_shapes=[
            pltpu.VMEM((rows_local, n), jnp.float32),
            pltpu.VMEM((2, RAW_ROWS, n), jnp.float32),
            pltpu.VMEM((N_DEV, 1, n), jnp.float32),
            pltpu.SemaphoreType.DMA((n_pieces,)),
            pltpu.SemaphoreType.DMA((2,)),
            pltpu.SemaphoreType.DMA((2,)),
            pltpu.SemaphoreType.DMA((4,)),
            pltpu.SemaphoreType.DMA((4,)),
        ],
        compiler_params=pltpu.CompilerParams(
            collective_id=0,
            vmem_limit_bytes=40 * 1024 * 1024,
            disable_semaphore_checks=True,
        ),
    )(x)
```

```python
import jax
import jax.numpy as jnp
from jax import lax
from jax.experimental import pallas as pl
from jax.experimental.pallas import tpu as pltpu

N_DEV = 4
MESH = pl.DeviceIdType.MESH

LANE = 128
RAW_ROWS = 208
BIG_CHUNK = 512
TAIL_CHUNKS = (256, 128, 64, 32, 16, 16)
NARROW_CHUNKS = (224, 32)
RAW_WAIT_BACK = 4


def _pieces(rows_local, n):
    wide_cols = n - LANE
    split0 = rows_local - sum(NARROW_CHUNKS)
    sizes, rest = [], split0 - sum(TAIL_CHUNKS)
    while rest > 0:
        sizes.append(min(BIG_CHUNK, rest))
        rest -= sizes[-1]
    pieces, row = [(split0, sum(NARROW_CHUNKS), 0, wide_cols)], 0
    for size in sizes + list(TAIL_CHUNKS):
        pieces.append((row, size, 0, n))
        row += size
    for size in NARROW_CHUNKS:
        pieces.append((row, size, wide_cols, LANE))
        row += size
    return pieces


def _colsum8(v):
    return jnp.sum(v.reshape(v.shape[0] // 8, 8, v.shape[1]), axis=0)


def _tree_add8(acc, v):
    parts = [acc] + [v[i:i + 8] for i in range(0, v.shape[0], 8)]
    while len(parts) > 1:
        pairs = [parts[i] + parts[i + 1] for i in range(0, len(parts) - 1, 2)]
        parts = pairs + parts[len(parts) - len(parts) % 2:]
    return parts[0]


def pallas_dist_mean_ax0_shard0_i_m4096_n1024_kernel(x: jax.Array):
    m_per, n = x.shape
    rows_local = m_per - 2 * RAW_ROWS
    wide_cols = n - LANE
    pieces = _pieces(rows_local, n)
    n_pieces = len(pieces)
    last_wide = n_pieces - 1 - len(NARROW_CHUNKS)
    inv_rows = 1.0 / (m_per * N_DEV)

    def body(x_hbm, out_ref, buf, raw_buf, comm,
             copy_sems, raw_send_sems, raw_recv_sems, send_sems, recv_sems):
        my = lax.axis_index("i")

        def peer(d):
            return ((my + d) % N_DEV,)

        def local_copy(p):
            r0, rn, c0, cn = pieces[p]
            return pltpu.make_async_copy(
                x_hbm.at[pl.ds(r0, rn), pl.ds(c0, cn)],
                buf.at[pl.ds(r0, rn), pl.ds(c0, cn)],
                copy_sems.at[p],
            )

        def partial_msg(d, k, c0, cn):
            return pltpu.make_async_remote_copy(
                src_ref=comm.at[0, :, pl.ds(c0, cn)],
                dst_ref=comm.at[d, :, pl.ds(c0, cn)],
                send_sem=send_sems.at[k],
                recv_sem=recv_sems.at[k],
                device_id=peer(d),
                device_id_type=MESH,
            )

        local_copy(0).start()
        barrier = pltpu.get_barrier_semaphore()
        for d in (1, 3, 2):
            pl.semaphore_signal(barrier, inc=1, device_id=peer(d), device_id_type=MESH)
        for p in range(1, n_pieces):
            local_copy(p).start()
        pl.semaphore_wait(barrier, N_DEV - 1)

        raw = []
        for b, d in enumerate((1, 3)):
            rd = pltpu.make_async_remote_copy(
                src_ref=x_hbm.at[pl.ds(rows_local + b * RAW_ROWS, RAW_ROWS), :],
                dst_ref=raw_buf.at[b],
                send_sem=raw_send_sems.at[b],
                recv_sem=raw_recv_sems.at[b],
                device_id=peer(d),
                device_id_type=MESH,
            )
            rd.start()
            raw.append(rd)

        to_next = partial_msg(1, 0, 0, n)
        to_prev = partial_msg(3, 1, 0, n)
        to_diag_wide = partial_msg(2, 2, 0, wide_cols)
        to_diag_last = partial_msg(2, 3, wide_cols, LANE)

        def add_rows(acc_wide, acc_last, rows):
            s = _colsum8(rows)
            return acc_wide + s[:, :wide_cols], acc_last + s[:, wide_cols:]

        acc_wide = jnp.zeros((8, wide_cols), jnp.float32)
        acc_last = jnp.zeros((8, LANE), jnp.float32)
        for p, (r0, rn, c0, cn) in enumerate(pieces):
            local_copy(p).wait()
            piece = buf[pl.ds(r0, rn), pl.ds(c0, cn)]
            if cn == n:
                acc_wide, acc_last = add_rows(acc_wide, acc_last, piece)
            elif c0 == 0:
                acc_wide = acc_wide + _colsum8(piece)
            else:
                acc_last = _tree_add8(acc_last, piece)
            if p == last_wide - RAW_WAIT_BACK:
                for b, rd in enumerate(raw):
                    rd.wait_recv()
                    acc_wide, acc_last = add_rows(acc_wide, acc_last, raw_buf[b])
                for rd in raw:
                    rd.wait_send()
            if p == last_wide:
                comm[0, :, pl.ds(0, wide_cols)] = jnp.sum(acc_wide, axis=0, keepdims=True)
                to_diag_wide.start()
        comm[0, :, pl.ds(wide_cols, LANE)] = jnp.sum(acc_last, axis=0, keepdims=True)
        to_diag_last.start()
        to_next.start()
        to_prev.start()

        for msg in (to_diag_wide, to_diag_last, to_next, to_prev):
            msg.wait_send()
        to_next.wait_recv()
        to_prev.wait_recv()
        near = (comm[0] + comm[1]) + comm[3]
        to_diag_wide.wait_recv()
        to_diag_last.wait_recv()
        out_ref[...] = (near + comm[2]) * inv_rows

    params = dict(collective_id=0, vmem_limit_bytes=40 * 1024 * 1024)
    if hasattr(pltpu.CompilerParams, "disable_semaphore_checks"):
        params["disable_semaphore_checks"] = True

    return pl.pallas_call(
        body,
        out_shape=jax.ShapeDtypeStruct((1, n), jnp.float32),
        in_specs=[pl.BlockSpec(memory_space=pl.ANY)],
        out_specs=pl.BlockSpec(memory_space=pltpu.VMEM),
        scratch_shapes=[
            pltpu.VMEM((rows_local, n), jnp.float32),
            pltpu.VMEM((2, RAW_ROWS, n), jnp.float32),
            pltpu.VMEM((N_DEV, 1, n), jnp.float32),
            pltpu.SemaphoreType.DMA((n_pieces,)),
            pltpu.SemaphoreType.DMA((2,)),
            pltpu.SemaphoreType.DMA((2,)),
            pltpu.SemaphoreType.DMA((4,)),
            pltpu.SemaphoreType.DMA((4,)),
        ],
        compiler_params=pltpu.CompilerParams(**params),
    )(x)
```

```python
import jax
import jax.numpy as jnp
from jax import lax
from jax.experimental import pallas as pl
from jax.experimental.pallas import tpu as pltpu

N_DEV = 4
MESH = pl.DeviceIdType.MESH

LANE = 128
RAW_ROWS = 208
BIG_CHUNK = 512
TAIL_CHUNKS = (256, 128, 64, 32, 16, 16)
NARROW_CHUNKS = (224, 32)
RAW_WAIT_BACK = 4


def _chunks(sizes):
    return [(sum(sizes[:i]), size) for i, size in enumerate(sizes)]


def _colsum8(v):
    return jnp.sum(v.reshape(v.shape[0] // 8, 8, v.shape[1]), axis=0)


def _tree_add8(acc, v):
    parts = [acc] + [v[i:i + 8] for i in range(0, v.shape[0], 8)]
    while len(parts) > 1:
        pairs = [parts[i] + parts[i + 1] for i in range(0, len(parts) - 1, 2)]
        parts = pairs + parts[len(parts) - len(parts) % 2:]
    return parts[0]


def pallas_dist_mean_ax0_shard0_i_m4096_n1024_kernel(x: jax.Array):
    m_per, n = x.shape
    wide = n - LANE
    split_rows = sum(NARROW_CHUNKS)
    full_rows = m_per - 2 * RAW_ROWS - split_rows
    raw0 = full_rows + split_rows
    n_big, rest = divmod(full_rows - sum(TAIL_CHUNKS), BIG_CHUNK)
    full_chunks = _chunks([BIG_CHUNK] * n_big + [rest] * (rest > 0) + list(TAIL_CHUNKS))
    narrow_chunks = _chunks(list(NARROW_CHUNKS))
    n_full = len(full_chunks)
    inv_rows = 1.0 / (m_per * N_DEV)

    def body(x_hbm, out_ref, full_buf, wide_buf, narrow_buf, raw_buf, comm,
             full_sems, wide_sem, narrow_sems, raw_send_sems, raw_recv_sems,
             send_sems, recv_sems):
        my = lax.axis_index("i")

        def peer(d):
            return ((my + d) % N_DEV,)

        wide_copy = pltpu.make_async_copy(
            x_hbm.at[pl.ds(full_rows, split_rows), pl.ds(0, wide)], wide_buf, wide_sem)
        full_copies = [
            pltpu.make_async_copy(
                x_hbm.at[pl.ds(r0, rn), :], full_buf.at[pl.ds(r0, rn), :], full_sems.at[c])
            for c, (r0, rn) in enumerate(full_chunks)
        ]
        narrow_copies = [
            pltpu.make_async_copy(
                x_hbm.at[pl.ds(full_rows + r0, rn), pl.ds(wide, LANE)],
                narrow_buf.at[pl.ds(r0, rn), :], narrow_sems.at[c])
            for c, (r0, rn) in enumerate(narrow_chunks)
        ]
        raw_copies = [
            pltpu.make_async_remote_copy(
                src_ref=x_hbm.at[pl.ds(raw0 + b * RAW_ROWS, RAW_ROWS), :],
                dst_ref=raw_buf.at[b],
                send_sem=raw_send_sems.at[b],
                recv_sem=raw_recv_sems.at[b],
                device_id=peer(d),
                device_id_type=MESH,
            )
            for b, d in enumerate((1, 3))
        ]

        def partial_msg(d, k, c0, cn):
            return pltpu.make_async_remote_copy(
                src_ref=comm.at[0, :, pl.ds(c0, cn)],
                dst_ref=comm.at[d, :, pl.ds(c0, cn)],
                send_sem=send_sems.at[k],
                recv_sem=recv_sems.at[k],
                device_id=peer(d),
                device_id_type=MESH,
            )

        to_next = partial_msg(1, 0, 0, n)
        to_prev = partial_msg(3, 1, 0, n)
        to_diag_wide = partial_msg(2, 2, 0, wide)
        to_diag_narrow = partial_msg(2, 3, wide, LANE)

        wide_copy.start()
        barrier = pltpu.get_barrier_semaphore()
        for d in (1, 3, 2):
            pl.semaphore_signal(barrier, inc=1, device_id=peer(d), device_id_type=MESH)
        for cp in full_copies:
            cp.start()
        pl.semaphore_wait(barrier, N_DEV - 1)
        for cp in raw_copies:
            cp.start()

        wide_copy.wait()
        for cp in narrow_copies:
            cp.start()
        acc_split = _colsum8(wide_buf[...])
        acc = jnp.zeros((8, n), jnp.float32)
        for c, (r0, rn) in enumerate(full_chunks):
            full_copies[c].wait()
            acc = acc + _colsum8(full_buf[pl.ds(r0, rn), :])
            if c == 0:
                acc = jnp.concatenate([acc[:, :wide] + acc_split, acc[:, wide:]], axis=1)
            if c == n_full - 1 - RAW_WAIT_BACK:
                for b, cp in enumerate(raw_copies):
                    cp.wait_recv()
                    acc = acc + _colsum8(raw_buf[b])
                for cp in raw_copies:
                    cp.wait_send()
        comm[0, :, pl.ds(0, wide)] = jnp.sum(acc[:, :wide], axis=0, keepdims=True)
        to_diag_wide.start()

        acc_narrow = acc[:, wide:]
        for c, (r0, rn) in enumerate(narrow_chunks):
            narrow_copies[c].wait()
            acc_narrow = _tree_add8(acc_narrow, narrow_buf[pl.ds(r0, rn), :])
        comm[0, :, pl.ds(wide, LANE)] = jnp.sum(acc_narrow, axis=0, keepdims=True)
        to_diag_narrow.start()
        to_next.start()
        to_prev.start()

        for msg in (to_diag_wide, to_diag_narrow, to_next, to_prev):
            msg.wait_send()
        to_next.wait_recv()
        to_prev.wait_recv()
        near = (comm[0] + comm[1]) + comm[3]
        to_diag_wide.wait_recv()
        to_diag_narrow.wait_recv()
        out_ref[...] = (near + comm[2]) * inv_rows

    params = dict(collective_id=0, vmem_limit_bytes=40 * 1024 * 1024)
    if hasattr(pltpu.CompilerParams, "disable_semaphore_checks"):
        params["disable_semaphore_checks"] = True

    return pl.pallas_call(
        body,
        out_shape=jax.ShapeDtypeStruct((1, n), jnp.float32),
        in_specs=[pl.BlockSpec(memory_space=pl.ANY)],
        out_specs=pl.BlockSpec(memory_space=pltpu.VMEM),
        scratch_shapes=[
            pltpu.VMEM((full_rows, n), jnp.float32),
            pltpu.VMEM((split_rows, wide), jnp.float32),
            pltpu.VMEM((split_rows, LANE), jnp.float32),
            pltpu.VMEM((2, RAW_ROWS, n), jnp.float32),
            pltpu.VMEM((N_DEV, 1, n), jnp.float32),
            pltpu.SemaphoreType.DMA((n_full,)),
            pltpu.SemaphoreType.DMA,
            pltpu.SemaphoreType.DMA((len(NARROW_CHUNKS),)),
            pltpu.SemaphoreType.DMA((2,)),
            pltpu.SemaphoreType.DMA((2,)),
            pltpu.SemaphoreType.DMA((4,)),
            pltpu.SemaphoreType.DMA((4,)),
        ],
        compiler_params=pltpu.CompilerParams(**params),
    )(x)
```

```python
import jax
import jax.numpy as jnp
from jax import lax
from jax.experimental import pallas as pl
from jax.experimental.pallas import tpu as pltpu

N_DEV = 4
MESH = pl.DeviceIdType.MESH

LANE = 128
RAW_ROWS = 208
BIG_CHUNK = 512
TAIL_CHUNKS = (256, 128, 64, 32, 16, 16)
NARROW_CHUNKS = (224, 32)
RAW_WAIT_BACK = 4


def _chunks(sizes):
    return [(sum(sizes[:i]), size) for i, size in enumerate(sizes)]


def _colsum8(v):
    return jnp.sum(v.reshape(v.shape[0] // 8, 8, v.shape[1]), axis=0)


def _tree_add8(acc, v):
    parts = [acc] + [v[i:i + 8] for i in range(0, v.shape[0], 8)]
    while len(parts) > 1:
        pairs = [parts[i] + parts[i + 1] for i in range(0, len(parts) - 1, 2)]
        parts = pairs + parts[len(parts) - len(parts) % 2:]
    return parts[0]


def pallas_dist_mean_ax0_shard0_i_m4096_n1024_kernel(x: jax.Array):
    m_per, n = x.shape
    wide = n - LANE
    split_rows = sum(NARROW_CHUNKS)
    full_rows = m_per - 2 * RAW_ROWS - split_rows
    raw0 = full_rows + split_rows
    n_big, rest = divmod(full_rows - sum(TAIL_CHUNKS), BIG_CHUNK)
    full_chunks = _chunks([BIG_CHUNK] * n_big + [rest] * (rest > 0) + list(TAIL_CHUNKS))
    narrow_chunks = _chunks(list(NARROW_CHUNKS))
    n_full = len(full_chunks)
    inv_rows = 1.0 / (m_per * N_DEV)

    def body(x_hbm, out_ref, full_buf, wide_buf, narrow_buf, raw_buf, comm,
             full_sems, wide_sem, narrow_sems, raw_send_sems, raw_recv_sems,
             send_sems, recv_sems):
        my = lax.axis_index("i")

        def peer(d):
            return ((my + d) % N_DEV,)

        wide_copy = pltpu.make_async_copy(
            x_hbm.at[pl.ds(full_rows, split_rows), pl.ds(0, wide)], wide_buf, wide_sem)
        full_copies = [
            pltpu.make_async_copy(
                x_hbm.at[pl.ds(r0, rn), :], full_buf.at[pl.ds(r0, rn), :], full_sems.at[c])
            for c, (r0, rn) in enumerate(full_chunks)
        ]
        narrow_copies = [
            pltpu.make_async_copy(
                x_hbm.at[pl.ds(full_rows + r0, rn), pl.ds(wide, LANE)],
                narrow_buf.at[pl.ds(r0, rn), :], narrow_sems.at[c])
            for c, (r0, rn) in enumerate(narrow_chunks)
        ]
        raw_copies = [
            pltpu.make_async_remote_copy(
                src_ref=x_hbm.at[pl.ds(raw0 + b * RAW_ROWS, RAW_ROWS), :],
                dst_ref=raw_buf.at[b],
                send_sem=raw_send_sems.at[b],
                recv_sem=raw_recv_sems.at[b],
                device_id=peer(d),
                device_id_type=MESH,
            )
            for b, d in enumerate((1, 3))
        ]

        def partial_msg(d, k, c0, cn):
            return pltpu.make_async_remote_copy(
                src_ref=comm.at[0, :, pl.ds(c0, cn)],
                dst_ref=comm.at[d, :, pl.ds(c0, cn)],
                send_sem=send_sems.at[k],
                recv_sem=recv_sems.at[k],
                device_id=peer(d),
                device_id_type=MESH,
            )

        to_next = partial_msg(1, 0, 0, n)
        to_prev = partial_msg(3, 1, 0, n)
        to_diag_wide = partial_msg(2, 2, 0, wide)
        to_diag_narrow = partial_msg(2, 3, wide, LANE)

        wide_copy.start()
        barrier = pltpu.get_barrier_semaphore()
        for d in (1, 3, 2):
            pl.semaphore_signal(barrier, inc=1, device_id=peer(d), device_id_type=MESH)
        for cp in full_copies:
            cp.start()
        pl.semaphore_wait(barrier, N_DEV - 1)
        for cp in raw_copies:
            cp.start()

        wide_copy.wait()
        for cp in narrow_copies:
            cp.start()
        acc_split = _colsum8(wide_buf[...])
        acc = jnp.zeros((8, n), jnp.float32)
        for c, (r0, rn) in enumerate(full_chunks):
            full_copies[c].wait()
            acc = acc + _colsum8(full_buf[pl.ds(r0, rn), :])
            if c == 0:
                acc = jnp.concatenate([acc[:, :wide] + acc_split, acc[:, wide:]], axis=1)
            if c == n_full - 1 - RAW_WAIT_BACK:
                for b, cp in enumerate(raw_copies):
                    cp.wait_recv()
                    acc = acc + _colsum8(raw_buf[b])
        comm[0, :, pl.ds(0, wide)] = jnp.sum(acc[:, :wide], axis=0, keepdims=True)
        to_diag_wide.start()

        acc_narrow = acc[:, wide:]
        for c, (r0, rn) in enumerate(narrow_chunks):
            narrow_copies[c].wait()
            acc_narrow = _tree_add8(acc_narrow, narrow_buf[pl.ds(r0, rn), :])
        comm[0, :, pl.ds(wide, LANE)] = jnp.sum(acc_narrow, axis=0, keepdims=True)
        to_diag_narrow.start()
        to_next.start()
        to_prev.start()

        for cp in raw_copies + [to_diag_wide, to_diag_narrow, to_next, to_prev]:
            cp.wait_send()
        to_next.wait_recv()
        to_prev.wait_recv()
        near = (comm[0] + comm[1]) + comm[3]
        to_diag_wide.wait_recv()
        to_diag_narrow.wait_recv()
        out_ref[...] = (near + comm[2]) * inv_rows

    params = dict(collective_id=0, vmem_limit_bytes=40 * 1024 * 1024)
    if hasattr(pltpu.CompilerParams, "disable_semaphore_checks"):
        params["disable_semaphore_checks"] = True

    return pl.pallas_call(
        body,
        out_shape=jax.ShapeDtypeStruct((1, n), jnp.float32),
        in_specs=[pl.BlockSpec(memory_space=pl.ANY)],
        out_specs=pl.BlockSpec(memory_space=pltpu.VMEM),
        scratch_shapes=[
            pltpu.VMEM((full_rows, n), jnp.float32),
            pltpu.VMEM((split_rows, wide), jnp.float32),
            pltpu.VMEM((split_rows, LANE), jnp.float32),
            pltpu.VMEM((2, RAW_ROWS, n), jnp.float32),
            pltpu.VMEM((N_DEV, 1, n), jnp.float32),
            pltpu.SemaphoreType.DMA((n_full,)),
            pltpu.SemaphoreType.DMA,
            pltpu.SemaphoreType.DMA((len(NARROW_CHUNKS),)),
            pltpu.SemaphoreType.DMA((2,)),
            pltpu.SemaphoreType.DMA((2,)),
            pltpu.SemaphoreType.DMA((4,)),
            pltpu.SemaphoreType.DMA((4,)),
        ],
        compiler_params=pltpu.CompilerParams(**params),
    )(x)
```
